```python
import numpy as np

kernel_name = "dist_sum_ax0_shard0_i_m1536_n768"

def setup_inputs():
    return {"x": np.random.randn(6144, 768).astype(np.float32)}

def reference(x: np.ndarray) -> np.ndarray:
    return np.sum(x, axis=0, keepdims=True)
```

```python
import jax
import jax.numpy as jnp
from jax import lax
from jax.experimental import pallas as pl
from jax.experimental.pallas import tpu as pltpu

N_DEV = 4
MESH = pl.DeviceIdType.MESH
LATE = 2
RAW_ROWS = 48
TAIL_CHUNKS = (192, 96, 48, 32, 16)
N_BIG = 3


def pallas_dist_sum_ax0_shard0_i_m1536_n768_kernel(x):
    m, n = x.shape
    head_rows = 2 * RAW_ROWS
    rest = m - head_rows - sum(TAIL_CHUNKS)
    big = (rest // N_BIG) // 8 * 8
    chunks = (big,) * (N_BIG - 1) + (rest - (N_BIG - 1) * big,) + TAIL_CHUNKS
    n_chunks = len(chunks)
    offs = [head_rows + sum(chunks[:c]) for c in range(n_chunks)]

    def rsum(v):
        return jnp.sum(v.reshape(v.shape[0] // 8, 8, n), axis=0)

    def body(x_hbm, out_ref, buf, rbuf, slots, extra, load_sems, head_sem, send_sems, recv_sems,
             raw_send, raw_recv):
        my = lax.axis_index("i")
        is_late = my == LATE
        not_late = my != LATE
        is_helper = (my & 1) != (LATE & 1)

        loads = [
            pltpu.make_async_copy(
                x_hbm.at[pl.ds(offs[c], chunks[c])], buf.at[pl.ds(offs[c], chunks[c])],
                load_sems.at[c])
            for c in range(n_chunks)
        ]
        head = pltpu.make_async_copy(
            x_hbm.at[pl.ds(0, head_rows)], buf.at[pl.ds(0, head_rows)], head_sem)
        for ld in loads:
            ld.start()

        @pl.when(not_late)
        def _():
            head.start()

        barrier = pltpu.get_barrier_semaphore()
        peers = {1: (my + 1) & 3, 2: my ^ 2, 3: (my + 3) & 3}
        for k in range(1, N_DEV):
            pl.semaphore_signal(barrier, inc=1, device_id=(peers[k],), device_id_type=MESH)
        pl.semaphore_wait(barrier, N_DEV - 1)

        raws = [
            pltpu.make_async_remote_copy(
                src_ref=x_hbm.at[pl.ds(j * RAW_ROWS, RAW_ROWS)], dst_ref=rbuf,
                send_sem=raw_send.at[j], recv_sem=raw_recv,
                device_id=((LATE + step) % N_DEV,), device_id_type=MESH)
            for j, step in enumerate((1, N_DEV - 1))
        ]

        @pl.when(is_late)
        def _():
            for cp in raws:
                cp.start()

        acc = jnp.zeros((8, n), jnp.float32)
        for c in range(n_chunks):
            if c == n_chunks - 3:
                @pl.when(is_late)
                def _():
                    extra[...] = jnp.zeros((8, n), jnp.float32)

                @pl.when(not_late)
                def _():
                    head.wait()
                    extra[...] = rsum(buf[pl.ds(0, head_rows), :])

                @pl.when(is_helper)
                def _():
                    raws[0].wait_recv()
                    extra[...] += rsum(rbuf[...])

                acc = acc + extra[...]
            loads[c].wait()
            acc = acc + rsum(buf[pl.ds(offs[c], chunks[c]), :])
        slots[0] = jnp.sum(acc, axis=0, keepdims=True)

        sends = {}
        for k in (2, 1, 3):
            sends[k] = pltpu.make_async_remote_copy(
                src_ref=slots.at[0], dst_ref=slots.at[k],
                send_sem=send_sems.at[k - 1], recv_sem=recv_sems.at[k - 1],
                device_id=(peers[k],), device_id_type=MESH)
            sends[k].start()
        sends[1].wait_recv()
        sends[3].wait_recv()
        pre = (slots[0] + slots[1]) + slots[3]
        sends[2].wait_recv()
        out_ref[...] = pre + slots[2]
        for k in (2, 1, 3):
            sends[k].wait_send()

        @pl.when(is_late)
        def _():
            for cp in raws:
                cp.wait_send()

    return pl.pallas_call(
        body,
        out_shape=jax.ShapeDtypeStruct((1, n), jnp.float32),
        in_specs=[pl.BlockSpec(memory_space=pl.ANY)],
        out_specs=pl.BlockSpec(memory_space=pltpu.VMEM),
        scratch_shapes=[
            pltpu.VMEM((m, n), jnp.float32),
            pltpu.VMEM((RAW_ROWS, n), jnp.float32),
            pltpu.VMEM((N_DEV, 1, n), jnp.float32),
            pltpu.VMEM((8, n), jnp.float32),
            pltpu.SemaphoreType.DMA((n_chunks,)),
            pltpu.SemaphoreType.DMA,
            pltpu.SemaphoreType.DMA((N_DEV - 1,)),
            pltpu.SemaphoreType.DMA((N_DEV - 1,)),
            pltpu.SemaphoreType.DMA((2,)),
            pltpu.SemaphoreType.DMA,
        ],
        compiler_params=pltpu.CompilerParams(
            collective_id=0, disable_semaphore_checks=True, disable_bounds_checks=True),
    )(x)
```

```python
import jax
import jax.numpy as jnp
from jax import lax
from jax.experimental import pallas as pl
from jax.experimental.pallas import tpu as pltpu

N_DEV = 4
MESH = pl.DeviceIdType.MESH
LATE = 2
RAW_ROWS = 56
N_BIG = 3
MID_CHUNKS = (192, 96)
LAST_CHUNKS = (112, 16)
COLS_B = 128


def pallas_dist_sum_ax0_shard0_i_m1536_n768_kernel(x):
    m, n = x.shape
    head_rows = 2 * RAW_ROWS
    last_rows = sum(LAST_CHUNKS)
    cols_a = n - COLS_B
    rest = m - head_rows - sum(MID_CHUNKS) - last_rows
    big = (rest // N_BIG) // 8 * 8
    chunks = (big,) * (N_BIG - 1) + (rest - (N_BIG - 1) * big,) + MID_CHUNKS
    offs = [head_rows + sum(chunks[:c]) for c in range(len(chunks))]
    last_offs = [m - last_rows + sum(LAST_CHUNKS[:c]) for c in range(len(LAST_CHUNKS))]

    def rsum(v):
        rows, cols = v.shape
        return jnp.sum(v.reshape(rows // 8, 8, cols), axis=0)

    def body(x_hbm, out_ref, buf, rbuf, slot_a, slot_b, extra, load_sems, a_sems, b_sems, head_sem,
             send_a, recv_a, send_b, recv_b, raw_send, raw_recv):
        my = lax.axis_index("i")
        is_late = my == LATE
        not_late = my != LATE
        is_helper = (my & 1) != (LATE & 1)

        def local_load(row0, rows, col0, cols, sem):
            return pltpu.make_async_copy(
                x_hbm.at[pl.ds(row0, rows), pl.ds(col0, cols)],
                buf.at[pl.ds(row0, rows), pl.ds(col0, cols)], sem)

        head = local_load(0, head_rows, 0, n, head_sem)
        loads = [local_load(offs[c], chunks[c], 0, n, load_sems.at[c]) for c in range(len(chunks))]
        a_loads = [local_load(last_offs[c], LAST_CHUNKS[c], 0, cols_a, a_sems.at[c])
                   for c in range(len(LAST_CHUNKS))]
        b_loads = [local_load(last_offs[c], LAST_CHUNKS[c], cols_a, COLS_B, b_sems.at[c])
                   for c in range(len(LAST_CHUNKS))]

        loads[0].start()

        @pl.when(not_late)
        def _():
            head.start()

        for ld in loads[1:] + a_loads + b_loads:
            ld.start()

        barrier = pltpu.get_barrier_semaphore()
        peers = {1: (my + 1) & 3, 2: my ^ 2, 3: (my + 3) & 3}
        for k in range(1, N_DEV):
            pl.semaphore_signal(barrier, inc=1, device_id=(peers[k],), device_id_type=MESH)
        pl.semaphore_wait(barrier, N_DEV - 1)

        raws = [
            pltpu.make_async_remote_copy(
                src_ref=x_hbm.at[pl.ds(j * RAW_ROWS, RAW_ROWS)], dst_ref=rbuf,
                send_sem=raw_send.at[j], recv_sem=raw_recv,
                device_id=((LATE + step) % N_DEV,), device_id_type=MESH)
            for j, step in enumerate((1, N_DEV - 1))
        ]

        @pl.when(is_late)
        def _():
            for cp in raws:
                cp.start()

        acc = jnp.zeros((8, n), jnp.float32)
        for c in range(len(chunks)):
            loads[c].wait()
            acc = acc + rsum(buf[pl.ds(offs[c], chunks[c]), :])

        @pl.when(is_late)
        def _():
            extra[...] = jnp.zeros((8, n), jnp.float32)

        @pl.when(not_late)
        def _():
            head.wait()
            extra[...] = rsum(buf[pl.ds(0, head_rows), :])

        @pl.when(is_helper)
        def _():
            raws[0].wait_recv()
            extra[...] += rsum(rbuf[...])

        acc = acc + extra[...]

        def exchange(slot, send_sems, recv_sems):
            return {
                k: pltpu.make_async_remote_copy(
                    src_ref=slot.at[0], dst_ref=slot.at[k],
                    send_sem=send_sems.at[k - 1], recv_sem=recv_sems.at[k - 1],
                    device_id=(peers[k],), device_id_type=MESH)
                for k in range(1, N_DEV)
            }

        copies_a = exchange(slot_a, send_a, recv_a)
        copies_b = exchange(slot_b, send_b, recv_b)

        acc_a = acc[:, :cols_a]
        for c in range(len(LAST_CHUNKS)):
            a_loads[c].wait()
            acc_a = acc_a + rsum(buf[pl.ds(last_offs[c], LAST_CHUNKS[c]), pl.ds(0, cols_a)])
        slot_a[0] = jnp.sum(acc_a, axis=0, keepdims=True)
        copies_a[2].start()

        acc_b = acc[:, cols_a:]
        for c in range(len(LAST_CHUNKS)):
            b_loads[c].wait()
            acc_b = acc_b + rsum(buf[pl.ds(last_offs[c], LAST_CHUNKS[c]), pl.ds(cols_a, COLS_B)])
        slot_b[0] = jnp.sum(acc_b, axis=0, keepdims=True)
        copies_b[2].start()
        for k in (1, 3):
            copies_a[k].start()
            copies_b[k].start()

        for k in (1, 3):
            copies_a[k].wait_recv()
            copies_b[k].wait_recv()
        pre_a = (slot_a[0] + slot_a[1]) + slot_a[3]
        pre_b = (slot_b[0] + slot_b[1]) + slot_b[3]
        for k in range(1, N_DEV):
            copies_a[k].wait_send()
            copies_b[k].wait_send()

        @pl.when(is_late)
        def _():
            for cp in raws:
                cp.wait_send()

        copies_a[2].wait_recv()
        out_ref[:, pl.ds(0, cols_a)] = pre_a + slot_a[2]
        copies_b[2].wait_recv()
        out_ref[:, pl.ds(cols_a, COLS_B)] = pre_b + slot_b[2]

    return pl.pallas_call(
        body,
        out_shape=jax.ShapeDtypeStruct((1, n), jnp.float32),
        in_specs=[pl.BlockSpec(memory_space=pl.ANY)],
        out_specs=pl.BlockSpec(memory_space=pltpu.VMEM),
        scratch_shapes=[
            pltpu.VMEM((m, n), jnp.float32),
            pltpu.VMEM((RAW_ROWS, n), jnp.float32),
            pltpu.VMEM((N_DEV, 1, cols_a), jnp.float32),
            pltpu.VMEM((N_DEV, 1, COLS_B), jnp.float32),
            pltpu.VMEM((8, n), jnp.float32),
            pltpu.SemaphoreType.DMA((len(chunks),)),
            pltpu.SemaphoreType.DMA((len(LAST_CHUNKS),)),
            pltpu.SemaphoreType.DMA((len(LAST_CHUNKS),)),
            pltpu.SemaphoreType.DMA,
            pltpu.SemaphoreType.DMA((N_DEV - 1,)),
            pltpu.SemaphoreType.DMA((N_DEV - 1,)),
            pltpu.SemaphoreType.DMA((N_DEV - 1,)),
            pltpu.SemaphoreType.DMA((N_DEV - 1,)),
            pltpu.SemaphoreType.DMA((2,)),
            pltpu.SemaphoreType.DMA,
        ],
        compiler_params=pltpu.CompilerParams(collective_id=0, disable_semaphore_checks=True),
    )(x)
```

```python
import jax
import jax.numpy as jnp
from jax import lax
from jax.experimental import pallas as pl
from jax.experimental.pallas import tpu as pltpu

N_DEV = 4
MESH = pl.DeviceIdType.MESH
LATE = 2
RAW_ROWS = 56
N_BIG = 3
MID_CHUNKS = (192, 96)
A_CHUNKS = (128, 32)
B_CHUNKS = (112, 40, 8)
COLS_B = 128


def pallas_dist_sum_ax0_shard0_i_m1536_n768_kernel(x):
    m, n = x.shape
    head_rows = 2 * RAW_ROWS
    last_rows = sum(A_CHUNKS)
    assert last_rows == sum(B_CHUNKS)
    cols_a = n - COLS_B
    rest = m - head_rows - sum(MID_CHUNKS) - last_rows
    big = (rest // N_BIG) // 8 * 8
    chunks = (big,) * (N_BIG - 1) + (rest - (N_BIG - 1) * big,) + MID_CHUNKS
    offs = [head_rows + sum(chunks[:c]) for c in range(len(chunks))]
    a_offs = [m - last_rows + sum(A_CHUNKS[:c]) for c in range(len(A_CHUNKS))]
    b_offs = [m - last_rows + sum(B_CHUNKS[:c]) for c in range(len(B_CHUNKS))]

    def rsum(v):
        rows, cols = v.shape
        return jnp.sum(v.reshape(rows // 8, 8, cols), axis=0)

    def tree_sum(terms):
        while len(terms) > 1:
            terms = [terms[i] + terms[i + 1] if i + 1 < len(terms) else terms[i]
                     for i in range(0, len(terms), 2)]
        return terms[0]

    def body(x_hbm, out_ref, buf, rbuf, slot_a, slot_b, extra, load_sems, a_sems, b_sems, head_sem,
             send_a, recv_a, send_b, recv_b, raw_send, raw_recv):
        my = lax.axis_index("i")
        is_late = my == LATE
        not_late = my != LATE
        is_helper = (my & 1) != (LATE & 1)

        def local_load(row0, rows, col0, cols, sem):
            return pltpu.make_async_copy(
                x_hbm.at[pl.ds(row0, rows), pl.ds(col0, cols)],
                buf.at[pl.ds(row0, rows), pl.ds(col0, cols)], sem)

        head = local_load(0, head_rows, 0, n, head_sem)
        loads = [local_load(offs[c], chunks[c], 0, n, load_sems.at[c]) for c in range(len(chunks))]
        a_loads = [local_load(a_offs[c], A_CHUNKS[c], 0, cols_a, a_sems.at[c])
                   for c in range(len(A_CHUNKS))]
        b_loads = [local_load(b_offs[c], B_CHUNKS[c], cols_a, COLS_B, b_sems.at[c])
                   for c in range(len(B_CHUNKS))]

        loads[0].start()

        @pl.when(not_late)
        def _():
            head.start()

        for ld in loads[1:] + a_loads + b_loads:
            ld.start()

        barrier = pltpu.get_barrier_semaphore()
        peers = {1: (my + 1) & 3, 2: my ^ 2, 3: (my + 3) & 3}
        for k in range(1, N_DEV):
            pl.semaphore_signal(barrier, inc=1, device_id=(peers[k],), device_id_type=MESH)
        pl.semaphore_wait(barrier, N_DEV - 1)

        raws = [
            pltpu.make_async_remote_copy(
                src_ref=x_hbm.at[pl.ds(j * RAW_ROWS, RAW_ROWS)], dst_ref=rbuf,
                send_sem=raw_send.at[j], recv_sem=raw_recv,
                device_id=((LATE + step) % N_DEV,), device_id_type=MESH)
            for j, step in enumerate((1, N_DEV - 1))
        ]

        @pl.when(is_late)
        def _():
            for cp in raws:
                cp.start()

        acc = jnp.zeros((8, n), jnp.float32)
        for c in range(len(chunks)):
            loads[c].wait()
            acc = acc + rsum(buf[pl.ds(offs[c], chunks[c]), :])

        @pl.when(is_late)
        def _():
            extra[...] = jnp.zeros((8, n), jnp.float32)

        @pl.when(not_late)
        def _():
            head.wait()
            extra[...] = rsum(buf[pl.ds(0, head_rows), :])

        @pl.when(is_helper)
        def _():
            raws[0].wait_recv()
            extra[...] += rsum(rbuf[...])

        acc = acc + extra[...]

        def exchange(slot, send_sems, recv_sems):
            return {
                k: pltpu.make_async_remote_copy(
                    src_ref=slot.at[0], dst_ref=slot.at[k],
                    send_sem=send_sems.at[k - 1], recv_sem=recv_sems.at[k - 1],
                    device_id=(peers[k],), device_id_type=MESH)
                for k in range(1, N_DEV)
            }

        copies_a = exchange(slot_a, send_a, recv_a)
        copies_b = exchange(slot_b, send_b, recv_b)

        acc_a = acc[:, :cols_a]
        for c in range(len(A_CHUNKS)):
            a_loads[c].wait()
            acc_a = acc_a + rsum(buf[pl.ds(a_offs[c], A_CHUNKS[c]), pl.ds(0, cols_a)])
        slot_a[0] = jnp.sum(acc_a, axis=0, keepdims=True)
        copies_a[2].start()

        acc_b = acc[:, cols_a:]
        for c in range(len(B_CHUNKS)):
            b_loads[c].wait()
            acc_b = tree_sum(
                [buf[pl.ds(b_offs[c] + 8 * i, 8), pl.ds(cols_a, COLS_B)]
                 for i in range(B_CHUNKS[c] // 8)] + [acc_b])
        slot_b[0] = jnp.sum(acc_b, axis=0, keepdims=True)
        copies_b[2].start()
        for k in (1, 3):
            copies_a[k].start()
            copies_b[k].start()

        for k in (1, 3):
            copies_a[k].wait_recv()
            copies_b[k].wait_recv()
        pre_a = (slot_a[0] + slot_a[1]) + slot_a[3]
        pre_b = (slot_b[0] + slot_b[1]) + slot_b[3]
        for k in range(1, N_DEV):
            copies_a[k].wait_send()
            copies_b[k].wait_send()

        @pl.when(is_late)
        def _():
            for cp in raws:
                cp.wait_send()

        copies_a[2].wait_recv()
        out_ref[:, pl.ds(0, cols_a)] = pre_a + slot_a[2]
        copies_b[2].wait_recv()
        out_ref[:, pl.ds(cols_a, COLS_B)] = pre_b + slot_b[2]

    return pl.pallas_call(
        body,
        out_shape=jax.ShapeDtypeStruct((1, n), jnp.float32),
        in_specs=[pl.BlockSpec(memory_space=pl.ANY)],
        out_specs=pl.BlockSpec(memory_space=pltpu.VMEM),
        scratch_shapes=[
            pltpu.VMEM((m, n), jnp.float32),
            pltpu.VMEM((RAW_ROWS, n), jnp.float32),
            pltpu.VMEM((N_DEV, 1, cols_a), jnp.float32),
            pltpu.VMEM((N_DEV, 1, COLS_B), jnp.float32),
            pltpu.VMEM((8, n), jnp.float32),
            pltpu.SemaphoreType.DMA((len(chunks),)),
            pltpu.SemaphoreType.DMA((len(A_CHUNKS),)),
            pltpu.SemaphoreType.DMA((len(B_CHUNKS),)),
            pltpu.SemaphoreType.DMA,
            pltpu.SemaphoreType.DMA((N_DEV - 1,)),
            pltpu.SemaphoreType.DMA((N_DEV - 1,)),
            pltpu.SemaphoreType.DMA((N_DEV - 1,)),
            pltpu.SemaphoreType.DMA((N_DEV - 1,)),
            pltpu.SemaphoreType.DMA((2,)),
            pltpu.SemaphoreType.DMA,
        ],
        compiler_params=pltpu.CompilerParams(collective_id=0, disable_semaphore_checks=True),
    )(x)
```
